```python
import numpy as np

kernel_name = "dist_rope_attn_qseq_b2_sq128_d512_hq4_dh64"

def setup_inputs():
    x = np.random.randn(2, 512, 512).astype(np.float32)
    Wq = np.random.randn(512, 256).astype(np.float32) * 0.02
    Wk = np.random.randn(512, 256).astype(np.float32) * 0.02
    Wv = np.random.randn(512, 256).astype(np.float32) * 0.02
    Wo = np.random.randn(256, 512).astype(np.float32) * 0.02
    return {"x": x, "Wq": Wq, "Wk": Wk, "Wv": Wv, "Wo": Wo}

def reference(x, Wq, Wk, Wv, Wo):
    B, Sq, Hq, Dh = 2, 512, 4, 64
    inv = 1.0 / (10000.0 ** (np.arange(0, Dh, 2) / Dh))
    pos = np.arange(Sq)[:, None] * inv[None, :]
    cos = np.repeat(np.cos(pos), 2, axis=-1).astype(np.float32)
    sin = np.repeat(np.sin(pos), 2, axis=-1).astype(np.float32)
    def rot(t):
        t2 = t.reshape(B, Sq, Hq, Dh // 2, 2)
        t_r = np.stack([-t2[..., 1], t2[..., 0]], axis=-1).reshape(B, Sq, Hq, Dh)
        return t * cos[None, :, None, :] + t_r * sin[None, :, None, :]
    Q = rot((x @ Wq).reshape(B, Sq, Hq, Dh))
    K = rot((x @ Wk).reshape(B, Sq, Hq, Dh))
    V = (x @ Wv).reshape(B, Sq, Hq, Dh)
    s = np.einsum('bihd,bjhd->bhij', Q, K).astype(np.float32) * 0.125
    s_max = s.max(axis=-1, keepdims=True)
    w = np.exp(s - s_max)
    w = w / w.sum(axis=-1, keepdims=True)
    ctx = np.einsum('bhij,bjhd->bihd', w, V).reshape(B, Sq, Hq * Dh)
    return ctx @ Wo
```

```python
import math

import jax
import jax.numpy as jnp
from jax import lax
from jax.experimental import pallas as pl
from jax.experimental.pallas import tpu as pltpu

NDEV = 4
B = 2
S_LOC = 128
S_ALL = NDEV * S_LOC
D = 512
HQ = 4
DH = 64
HD = HQ * DH
LANES = 128

_NEG_LOG_THETA_2_OVER_DH = -2.0 * math.log(10000.0) / DH

T_K, T_Q, T_V = 0, 1, 2
OWN = NDEV - 1

SEM_K = 0
SEM_V = 1
SEM_Q = 2
SEM_C = 5
N_RECV_SEMS = 8


def pallas_dist_rope_attn_qseq_b2_sq128_d512_hq4_dh64_kernel(
    x: jax.Array,
    Wq: jax.Array,
    Wk: jax.Array,
    Wv: jax.Array,
    Wo: jax.Array,
):
    def body(x_hbm, wq_hbm, wk_hbm, wv_hbm, wo_hbm, out_ref,
             x_v, wq_v, wk_v, wv_v, wo_v,
             send_buf, recv_buf, p_buf, linv_buf, ctx_send, ctx_recv,
             load_sems, send_sem, recv_sems):
        me = lax.axis_index("i")
        my_b = me // 2
        my_hp = me % 2

        cp_x = pltpu.make_async_copy(x_hbm, x_v, load_sems.at[0])
        cp_wk = pltpu.make_async_copy(wk_hbm, wk_v, load_sems.at[0])
        cp_wq = pltpu.make_async_copy(wq_hbm, wq_v, load_sems.at[1])
        cp_wv = pltpu.make_async_copy(wv_hbm, wv_v, load_sems.at[2])
        cp_wo = pltpu.make_async_copy(wo_hbm, wo_v, load_sems.at[3])
        cp_x.start()
        cp_wk.start()
        cp_wq.start()
        cp_wv.start()
        cp_wo.start()

        barrier = pltpu.get_barrier_semaphore()
        for k in range(1, NDEV):
            pl.semaphore_signal(
                barrier, inc=1, device_id=((me + k) % NDEV,),
                device_id_type=pl.DeviceIdType.MESH)

        row = lax.broadcasted_iota(jnp.int32, (S_LOC, LANES), 0)
        lane = lax.broadcasted_iota(jnp.int32, (S_LOC, LANES), 1)
        pos = (me * S_LOC + row).astype(jnp.float32)
        freq = ((lane % DH) // 2).astype(jnp.float32)
        inv = jnp.exp(freq * _NEG_LOG_THETA_2_OVER_DH)
        ang = pos * inv
        cos_t = jnp.cos(ang)
        sin_t = jnp.sin(ang)
        even = (lane % 2) == 0
        sin_s = jnp.where(even, -sin_t, sin_t)

        def rope(t):
            t_next = pltpu.roll(t, LANES - 1, 1)
            t_prev = pltpu.roll(t, 1, 1)
            return t * cos_t + jnp.where(even, t_next, t_prev) * sin_s

        sends = []

        def send(src_ref, dst_ref, recv_sem, k):
            c = pltpu.make_async_remote_copy(
                src_ref=src_ref, dst_ref=dst_ref,
                send_sem=send_sem, recv_sem=recv_sem,
                device_id=((me + k) % NDEV,),
                device_id_type=pl.DeviceIdType.MESH)
            c.start()
            sends.append(c)

        def wait_landed(ref, sem):
            pltpu.make_async_copy(ref, ref, sem).wait()

        def project(xb, w_v, t, do_rope, scale):
            wb = w_v[...].astype(jnp.bfloat16)
            for hp in range(2):
                tt = jnp.dot(xb, wb[:, hp * LANES:(hp + 1) * LANES],
                             preferred_element_type=jnp.float32)
                for b in range(B):
                    piece = tt[b * S_LOC:(b + 1) * S_LOC, :]
                    if do_rope:
                        piece = rope(piece)
                    if scale is not None:
                        piece = piece * scale
                    send_buf[t, b, hp] = piece.astype(jnp.bfloat16)

        def scatter(t, shared_sem):
            for k in (2, 1, 3):
                d = (me + k) % NDEV
                sem = recv_sems.at[shared_sem if shared_sem is not None
                                   else SEM_Q + k - 1]
                send(send_buf.at[t, d // 2, d % 2], recv_buf.at[t, k - 1], sem, k)
            recv_buf[t, OWN] = send_buf[t, my_b, my_hp]

        cp_x.wait()
        cp_wk.wait()
        xb = x_v[...].reshape(B * S_LOC, D).astype(jnp.bfloat16)
        project(xb, wk_v, T_K, True, None)
        pl.semaphore_wait(barrier, NDEV - 1)
        scatter(T_K, SEM_K)

        cp_wq.wait()
        project(xb, wq_v, T_Q, True, 0.125)
        scatter(T_Q, None)

        cp_wv.wait()
        project(xb, wv_v, T_V, False, None)
        scatter(T_V, SEM_V)

        remote_slots = pl.ds(0, NDEV - 1)
        wait_landed(recv_buf.at[T_K, remote_slots], recv_sems.at[SEM_K])
        k_all = recv_buf[T_K].reshape(S_ALL, LANES)

        for j in (OWN, 0, 1, 2):
            if j != OWN:
                wait_landed(recv_buf.at[T_Q, j], recv_sems.at[SEM_Q + j])
            q = recv_buf[T_Q, j].astype(jnp.float32)
            for h in range(2):
                in_head = (lane >= h * DH) & (lane < (h + 1) * DH)
                qm = jnp.where(in_head, q, 0.0).astype(jnp.bfloat16)
                s = lax.dot_general(qm, k_all, (((1,), (1,)), ((), ())),
                                    preferred_element_type=jnp.float32)
                m = jnp.max(s, axis=-1, keepdims=True)
                e = jnp.exp(s - m)
                l = jnp.sum(e, axis=-1, keepdims=True)
                p_buf[h, j] = e.astype(jnp.bfloat16)
                linv_buf[h, j] = jnp.broadcast_to(1.0 / l, (S_LOC, LANES))

        wait_landed(recv_buf.at[T_V, remote_slots], recv_sems.at[SEM_V])
        v_all = recv_buf[T_V].reshape(S_ALL, LANES)

        for j in (1, 0, 2, OWN):
            o0 = jnp.dot(p_buf[0, j], v_all, preferred_element_type=jnp.float32)
            o1 = jnp.dot(p_buf[1, j], v_all, preferred_element_type=jnp.float32)
            ctx = jnp.where(lane < DH, o0 * linv_buf[0, j], o1 * linv_buf[1, j])
            ctx_send[j] = ctx.astype(jnp.bfloat16)
            if j != OWN:
                send(ctx_send.at[j], ctx_recv.at[me],
                     recv_sems.at[SEM_C + j], NDEV - (j + 1))
            else:
                ctx_recv[me] = ctx_send[OWN]

        cp_wo.wait()
        wob = wo_v[...].astype(jnp.bfloat16)
        for k in range(1, NDEV):
            wait_landed(ctx_recv.at[(me + k) % NDEV], recv_sems.at[SEM_C + k - 1])
        for b in range(B):
            o = jnp.dot(ctx_recv[2 * b], wob[0:LANES, :],
                        preferred_element_type=jnp.float32)
            o = o + jnp.dot(ctx_recv[2 * b + 1], wob[LANES:2 * LANES, :],
                            preferred_element_type=jnp.float32)
            out_ref[b] = o

        for c in sends:
            c.wait_send()

    return pl.pallas_call(
        body,
        out_shape=jax.ShapeDtypeStruct((B, S_LOC, D), jnp.float32),
        in_specs=[pl.BlockSpec(memory_space=pl.ANY)] * 5,
        out_specs=pl.BlockSpec(memory_space=pltpu.VMEM),
        scratch_shapes=[
            pltpu.VMEM((B, S_LOC, D), jnp.float32),
            pltpu.VMEM((D, HD), jnp.float32),
            pltpu.VMEM((D, HD), jnp.float32),
            pltpu.VMEM((D, HD), jnp.float32),
            pltpu.VMEM((HD, D), jnp.float32),
            pltpu.VMEM((3, B, 2, S_LOC, LANES), jnp.bfloat16),
            pltpu.VMEM((3, NDEV, S_LOC, LANES), jnp.bfloat16),
            pltpu.VMEM((2, NDEV, S_LOC, S_ALL), jnp.bfloat16),
            pltpu.VMEM((2, NDEV, S_LOC, LANES), jnp.float32),
            pltpu.VMEM((NDEV, S_LOC, LANES), jnp.bfloat16),
            pltpu.VMEM((NDEV, S_LOC, LANES), jnp.bfloat16),
            pltpu.SemaphoreType.DMA((4,)),
            pltpu.SemaphoreType.DMA,
            pltpu.SemaphoreType.DMA((N_RECV_SEMS,)),
        ],
        compiler_params=pltpu.CompilerParams(collective_id=0),
    )(x, Wq, Wk, Wv, Wo)
```
